```python
import numpy as np

kernel_name = "dist_ring_attn_i_s256_d64"

def setup_inputs():
    S, D = 1024, 64
    q = np.random.randn(S, D).astype(np.float32)
    k = np.random.randn(S, D).astype(np.float32)
    v = np.random.randn(S, D).astype(np.float32)
    return {"q": q, "k": k, "v": v}

def reference(q: np.ndarray, k: np.ndarray, v: np.ndarray) -> np.ndarray:
    D = q.shape[1]
    scores = q @ k.T / np.sqrt(D)
    scores_max = np.max(scores, axis=1, keepdims=True)
    weights = np.exp(scores - scores_max)
    weights = weights / np.sum(weights, axis=1, keepdims=True)
    return weights @ v
```

```python
import jax
import jax.numpy as jnp
from jax import lax
from jax.experimental import pallas as pl
from jax.experimental.pallas import tpu as pltpu

N_DEV = 4


def pallas_dist_ring_attn_i_s256_d64_kernel(
    q: jax.Array,
    k: jax.Array,
    v: jax.Array,
):
    s_per, d = q.shape
    scale = 1.0 / float(d) ** 0.5

    def body(q_hbm, k_hbm, v_hbm, out_ref,
             q_f32, k_f32, v_f32, kv_buf, load_sems, send_sems, recv_sems):
        my = lax.axis_index("i")

        ck = pltpu.make_async_copy(k_hbm, k_f32, load_sems.at[0])
        cv = pltpu.make_async_copy(v_hbm, v_f32, load_sems.at[1])
        cq = pltpu.make_async_copy(q_hbm, q_f32, load_sems.at[2])
        ck.start()
        cv.start()
        cq.start()

        barrier = pltpu.get_barrier_semaphore()
        for off in range(1, N_DEV):
            pl.semaphore_signal(
                barrier, inc=1,
                device_id=((my + off) % N_DEV,),
                device_id_type=pl.DeviceIdType.MESH,
            )

        ck.wait()
        cv.wait()
        kv_buf[0] = jnp.concatenate(
            [k_f32[...].astype(jnp.bfloat16), v_f32[...].astype(jnp.bfloat16)],
            axis=1,
        )

        pl.semaphore_wait(barrier, N_DEV - 1)

        rdmas = []
        for off in range(1, N_DEV):
            r = pltpu.make_async_remote_copy(
                src_ref=kv_buf.at[0],
                dst_ref=kv_buf.at[off],
                send_sem=send_sems.at[off - 1],
                recv_sem=recv_sems.at[off - 1],
                device_id=((my + off) % N_DEV,),
                device_id_type=pl.DeviceIdType.MESH,
            )
            r.start()
            rdmas.append(r)

        cq.wait()
        qs = (q_f32[...] * scale).astype(jnp.bfloat16)
        q_ext = jnp.concatenate([qs, jnp.zeros_like(qs)], axis=1)

        def block(slot, carry):
            kv = kv_buf[slot]
            s = lax.dot_general(
                q_ext, kv, (((1,), (1,)), ((), ())),
                preferred_element_type=jnp.float32,
            )
            m_blk = jnp.max(s, axis=1, keepdims=True)
            if carry is None:
                p = jnp.exp(s - m_blk)
                l = jnp.sum(p, axis=1, keepdims=True)
                acc = jnp.dot(p.astype(jnp.bfloat16), kv,
                              preferred_element_type=jnp.float32)
                return m_blk, l, acc
            m, l, acc = carry
            m_new = jnp.maximum(m, m_blk)
            alpha = jnp.exp(m - m_new)
            p = jnp.exp(s - m_new)
            l = alpha * l + jnp.sum(p, axis=1, keepdims=True)
            acc = alpha * acc + jnp.dot(p.astype(jnp.bfloat16), kv,
                                        preferred_element_type=jnp.float32)
            return m_new, l, acc

        carry = block(0, None)
        for off in (1, 3, 2):
            rdmas[off - 1].wait_recv()
            carry = block(off, carry)

        _, l, acc = carry
        out_ref[...] = acc[:, d:] / l

        for r in rdmas:
            r.wait_send()

    return pl.pallas_call(
        body,
        out_shape=jax.ShapeDtypeStruct((s_per, d), jnp.float32),
        in_specs=[pl.BlockSpec(memory_space=pl.ANY)] * 3,
        out_specs=pl.BlockSpec(memory_space=pltpu.VMEM),
        scratch_shapes=[
            pltpu.VMEM((s_per, d), jnp.float32),
            pltpu.VMEM((s_per, d), jnp.float32),
            pltpu.VMEM((s_per, d), jnp.float32),
            pltpu.VMEM((N_DEV, s_per, 2 * d), jnp.bfloat16),
            pltpu.SemaphoreType.DMA((3,)),
            pltpu.SemaphoreType.DMA((N_DEV - 1,)),
            pltpu.SemaphoreType.DMA((N_DEV - 1,)),
        ],
        compiler_params=pltpu.CompilerParams(collective_id=0),
    )(q, k, v)
```

```python
import jax
import jax.numpy as jnp
from jax import lax
from jax.experimental import pallas as pl
from jax.experimental.pallas import tpu as pltpu

N_DEV = 4

_OWN, _LEFT, _RIGHT, _DIAG = 0, 1, 2, 3


def pallas_dist_ring_attn_i_s256_d64_kernel(
    q: jax.Array,
    k: jax.Array,
    v: jax.Array,
):
    s_per, d = q.shape
    half = s_per // 2
    scale = 1.0 / float(d) ** 0.5

    def body(q_hbm, k_hbm, v_hbm, out_hbm,
             q_f32, k_f32, v_f32, out_buf, kv_buf,
             load_sems, send_sems, recv_sems):
        my = lax.axis_index("i")
        left = (my + N_DEV - 1) % N_DEV
        right = (my + 1) % N_DEV

        ck = pltpu.make_async_copy(k_hbm, k_f32, load_sems.at[0])
        cv = pltpu.make_async_copy(v_hbm, v_f32, load_sems.at[1])
        cq = pltpu.make_async_copy(q_hbm, q_f32, load_sems.at[2])
        ck.start()
        cv.start()
        cq.start()

        barrier = pltpu.get_barrier_semaphore()
        for nbr in (left, right):
            pl.semaphore_signal(
                barrier, inc=1, device_id=(nbr,),
                device_id_type=pl.DeviceIdType.MESH,
            )

        ck.wait()
        cv.wait()
        for h in range(2):
            cols = pl.ds(h * half, half)
            kv_buf[_OWN, h, :d, :] = k_f32[:, cols].astype(jnp.bfloat16)
            kv_buf[_OWN, h, d:, :] = v_f32[:, cols].astype(jnp.bfloat16)

        pl.semaphore_wait(barrier, 2)

        def rdma(idx, src_slot, dst_slot, h, target):
            return pltpu.make_async_remote_copy(
                src_ref=kv_buf.at[src_slot, h],
                dst_ref=kv_buf.at[dst_slot, h],
                send_sem=send_sems.at[idx],
                recv_sem=recv_sems.at[idx],
                device_id=(target,),
                device_id_type=pl.DeviceIdType.MESH,
            )

        to_r0 = rdma(0, _OWN, _LEFT, 0, right)
        to_l1 = rdma(1, _OWN, _RIGHT, 1, left)
        to_r1 = rdma(2, _OWN, _LEFT, 1, right)
        to_l0 = rdma(3, _OWN, _RIGHT, 0, left)
        for r in (to_r0, to_l1, to_r1, to_l0):
            r.start()
        fwd_r0 = rdma(4, _LEFT, _DIAG, 0, right)
        fwd_l1 = rdma(5, _RIGHT, _DIAG, 1, left)

        cq.wait()
        qt = (q_f32[...] * scale).astype(jnp.bfloat16)

        def block(slot, h, carry):
            kt = kv_buf[slot, h, :d, :]
            vt = kv_buf[slot, h, d:, :]
            st = lax.dot_general(
                kt, qt, (((0,), (0,)), ((), ())),
                preferred_element_type=jnp.float32,
            )
            m_blk = jnp.max(st, axis=0, keepdims=True)
            if carry is None:
                pt = jnp.exp(st - m_blk)
                l = jnp.sum(pt, axis=0, keepdims=True)
                acc = jnp.dot(vt, pt.astype(jnp.bfloat16),
                              preferred_element_type=jnp.float32)
                return m_blk, l, acc
            m, l, acc = carry
            m_new = jnp.maximum(m, m_blk)
            alpha = jnp.exp(m - m_new)
            pt = jnp.exp(st - m_new)
            l = alpha * l + jnp.sum(pt, axis=0, keepdims=True)
            acc = alpha * acc + jnp.dot(vt, pt.astype(jnp.bfloat16),
                                        preferred_element_type=jnp.float32)
            return m_new, l, acc

        carry = block(_OWN, 0, None)
        carry = block(_OWN, 1, carry)

        to_r0.wait_recv()
        fwd_r0.start()
        to_l1.wait_recv()
        fwd_l1.start()
        carry = block(_LEFT, 0, carry)
        carry = block(_RIGHT, 1, carry)

        to_r1.wait_recv()
        carry = block(_LEFT, 1, carry)
        to_l0.wait_recv()
        carry = block(_RIGHT, 0, carry)

        fwd_r0.wait_recv()
        carry = block(_DIAG, 0, carry)
        fwd_l1.wait_recv()
        carry = block(_DIAG, 1, carry)

        _, l, acc = carry
        out_buf[...] = acc / l
        co = pltpu.make_async_copy(out_buf, out_hbm, load_sems.at[0])
        co.start()

        for r in (to_r0, to_l1, to_r1, to_l0, fwd_r0, fwd_l1):
            r.wait_send()
        co.wait()

    out_t = pl.pallas_call(
        body,
        out_shape=jax.ShapeDtypeStruct((d, s_per), jnp.float32),
        in_specs=[pl.BlockSpec(memory_space=pl.ANY)] * 3,
        out_specs=pl.BlockSpec(memory_space=pl.ANY),
        scratch_shapes=[
            pltpu.VMEM((d, s_per), jnp.float32),
            pltpu.VMEM((d, s_per), jnp.float32),
            pltpu.VMEM((d, s_per), jnp.float32),
            pltpu.VMEM((d, s_per), jnp.float32),
            pltpu.VMEM((N_DEV, 2, 2 * d, half), jnp.bfloat16),
            pltpu.SemaphoreType.DMA((3,)),
            pltpu.SemaphoreType.DMA((6,)),
            pltpu.SemaphoreType.DMA((6,)),
        ],
        compiler_params=pltpu.CompilerParams(collective_id=0),
    )(q.T, k.T, v.T)
    return out_t.T
```

```python
import jax
import jax.numpy as jnp
from jax import lax
from jax.experimental import pallas as pl
from jax.experimental.pallas import tpu as pltpu

N_DEV = 4

_OWN, _LEFT, _RIGHT, _DIAG = 0, 1, 2, 3


def pallas_dist_ring_attn_i_s256_d64_kernel(
    q: jax.Array,
    k: jax.Array,
    v: jax.Array,
):
    s_per, d = q.shape
    half = s_per // 2
    scale = 1.0 / float(d) ** 0.5

    def body(q_hbm, k_hbm, v_hbm, out_ref,
             q_f32, k_f32, v_f32, kv_buf,
             load_sems, send_sems, recv_sems):
        my = lax.axis_index("i")
        left = (my + N_DEV - 1) % N_DEV
        right = (my + 1) % N_DEV

        ck = pltpu.make_async_copy(k_hbm, k_f32, load_sems.at[0])
        cv = pltpu.make_async_copy(v_hbm, v_f32, load_sems.at[1])
        cq = pltpu.make_async_copy(q_hbm, q_f32, load_sems.at[2])
        ck.start()
        cv.start()
        cq.start()

        barrier = pltpu.get_barrier_semaphore()
        for nbr in (left, right):
            pl.semaphore_signal(
                barrier, inc=1, device_id=(nbr,),
                device_id_type=pl.DeviceIdType.MESH,
            )

        ck.wait()
        cv.wait()
        for h in range(2):
            cols = pl.ds(h * half, half)
            kv_buf[_OWN, h, :d, :] = k_f32[:, cols].astype(jnp.bfloat16)
            kv_buf[_OWN, h, d:, :] = v_f32[:, cols].astype(jnp.bfloat16)

        pl.semaphore_wait(barrier, 2)

        def rdma(idx, src_slot, dst_slot, h, target):
            return pltpu.make_async_remote_copy(
                src_ref=kv_buf.at[src_slot, h],
                dst_ref=kv_buf.at[dst_slot, h],
                send_sem=send_sems.at[idx],
                recv_sem=recv_sems.at[idx],
                device_id=(target,),
                device_id_type=pl.DeviceIdType.MESH,
            )

        to_r0 = rdma(0, _OWN, _LEFT, 0, right)
        to_l1 = rdma(1, _OWN, _RIGHT, 1, left)
        to_r1 = rdma(2, _OWN, _LEFT, 1, right)
        to_l0 = rdma(3, _OWN, _RIGHT, 0, left)
        for r in (to_r0, to_l1, to_r1, to_l0):
            r.start()
        fwd_r0 = rdma(4, _LEFT, _DIAG, 0, right)
        fwd_l1 = rdma(5, _RIGHT, _DIAG, 1, left)

        cq.wait()
        qt = (q_f32[...] * scale).astype(jnp.bfloat16)

        def block(slot, h, carry):
            kt = kv_buf[slot, h, :d, :]
            vt = kv_buf[slot, h, d:, :]
            st = lax.dot_general(
                kt, qt, (((0,), (0,)), ((), ())),
                preferred_element_type=jnp.float32,
            )
            m_blk = jnp.max(st, axis=0, keepdims=True)
            if carry is None:
                pt = jnp.exp(st - m_blk)
                l = jnp.sum(pt, axis=0, keepdims=True)
                acc = jnp.dot(vt, pt.astype(jnp.bfloat16),
                              preferred_element_type=jnp.float32)
                return m_blk, l, acc
            m, l, acc = carry
            m_new = jnp.maximum(m, m_blk)
            alpha = jnp.exp(m - m_new)
            pt = jnp.exp(st - m_new)
            l = alpha * l + jnp.sum(pt, axis=0, keepdims=True)
            acc = alpha * acc + jnp.dot(vt, pt.astype(jnp.bfloat16),
                                        preferred_element_type=jnp.float32)
            return m_new, l, acc

        carry = block(_OWN, 0, None)
        carry = block(_OWN, 1, carry)

        to_r0.wait_recv()
        fwd_r0.start()
        to_l1.wait_recv()
        fwd_l1.start()
        carry = block(_LEFT, 0, carry)
        carry = block(_RIGHT, 1, carry)

        to_r1.wait_recv()
        carry = block(_LEFT, 1, carry)
        to_l0.wait_recv()
        carry = block(_RIGHT, 0, carry)

        fwd_r0.wait_recv()
        carry = block(_DIAG, 0, carry)
        fwd_l1.wait_recv()
        carry = block(_DIAG, 1, carry)

        _, l, acc = carry
        out_ref[...] = acc / l

        for r in (to_r0, to_l1, to_r1, to_l0, fwd_r0, fwd_l1):
            r.wait_send()

    out_t = pl.pallas_call(
        body,
        out_shape=jax.ShapeDtypeStruct((d, s_per), jnp.float32),
        in_specs=[pl.BlockSpec(memory_space=pl.ANY)] * 3,
        out_specs=pl.BlockSpec(memory_space=pltpu.VMEM),
        scratch_shapes=[
            pltpu.VMEM((d, s_per), jnp.float32),
            pltpu.VMEM((d, s_per), jnp.float32),
            pltpu.VMEM((d, s_per), jnp.float32),
            pltpu.VMEM((N_DEV, 2, 2 * d, half), jnp.bfloat16),
            pltpu.SemaphoreType.DMA((3,)),
            pltpu.SemaphoreType.DMA((6,)),
            pltpu.SemaphoreType.DMA((6,)),
        ],
        compiler_params=pltpu.CompilerParams(collective_id=0),
    )(q.T, k.T, v.T)
    return out_t.T
```
